```python
import numpy as np

kernel_name = "dist_ag_xy_y_m65536_n1024"

def setup_inputs():
    return {"x": np.random.randn(131072, 1024).astype(np.float32)}

def reference(x: np.ndarray) -> np.ndarray:
    return x
```

```python
import numpy as np
import jax
import jax.numpy as jnp
from jax import lax
from jax.experimental import pallas as pl
from jax.experimental.pallas import tpu as pltpu


WORDS = 7
UNIT_BITS = 28


def _i32(v):
    return np.int32(v - (1 << 32) if v >= (1 << 31) else v)


def _shr(a, b):
    return lax.shift_right_logical(a, jnp.broadcast_to(jnp.asarray(b, jnp.int32), a.shape))


def _shl(a, b):
    return lax.shift_left(a, jnp.broadcast_to(jnp.asarray(b, jnp.int32), a.shape))


def _swap_bytes(a, b):
    t = (_shr(a, 8) ^ b) & _i32(0x00FF00FF)
    return a ^ _shl(t, 8), b ^ t


MSB = _i32(0x80808080)
LOW7 = _i32(0x7F7F7F7F)


def _bin_to_len(q):
    ge4 = (q + _i32(0x7C7C7C7C)) & MSB
    ge1 = (q + LOW7) & MSB
    return (q + _i32(0x04040404)) + _shr(ge4, 7) - _shr(ge1, 5)


def _zeros_to_bin(n):
    ge3 = (n + _i32(0x7D7D7D7D)) & MSB
    ge4 = (n + _i32(0x7C7C7C7C)) & MSB
    return (n + _i32(0x01010101)) - _shr(ge3 ^ ge4, 5) - _shr(ge4, 7)


def encode_unit(w, bias, pos):
    low, signs, group, glen = [], None, [], []
    long_code = None
    for i in range(4):
        lo, hi = _swap_bytes(bias - w[2 * i], bias - w[2 * i + 1])
        low.append(lo)
        s = hi & MSB
        signs = s if i == 0 else signs | _shr(s, i)
        ln = _bin_to_len(hi & LOW7)
        long_code = ln if i == 0 else long_code | ln
        l0, l1, l2, l3 = ln & 255, _shr(ln, 8) & 255, _shr(ln, 16) & 255, _shr(ln, 24)
        acc = _shl(jnp.ones_like(ln), l1) | 1
        acc = _shl(acc, l2) | 1
        acc = _shl(acc, l3) | 1
        group.append(acc)
        glen.append((l0 + l1) + (l2 + l3))
    lo, hi = group[0], None
    for i in range(1, 4):
        carry = _shr(lo, 32 - glen[i])
        hi = carry if hi is None else _shl(hi, glen[i]) | carry
        lo = _shl(lo, glen[i]) | group[i]
    total = (glen[0] + glen[1]) + (glen[2] + glen[3])
    end = pos + total
    bad = ((long_code & _i32(0xE0E0E0E0)) | ((glen[0] | glen[1] | glen[2] | glen[3]) & ~31)
           | ((total - 1) & ~63) | ((32 * WORDS - end) & _i32(0x80000000)))
    t = (-end) & 31
    u = 31 - t
    z0 = _shl(lo, t)
    z1 = _shl(hi, t) | _shr(_shr(lo, 1), u)
    z2 = _shr(_shr(hi, 1), u)
    last = end - 1
    zero = jnp.zeros_like(z0)
    out = {-2: z2, -1: z1, 0: z0}
    for step in (1, 2, 4):
        up = (last & (32 * step)) != 0
        lo_k = 0 if step == 4 else -2
        out = {k: jnp.where(up, out.get(k - step, zero), out.get(k, zero))
               for k in range(lo_k, min(max(out) + step, WORDS - 1) + 1)}
    return low, signs, [out[k] for k in range(WORDS)], end, bad


def decode_unit(low, signs, win, bias, pos):
    x = list(win)
    for step, keep in ((4, 6), (2, 4), (1, 3)):
        down = (pos & (32 * step)) != 0
        x = [jnp.where(down, x[k + step], x[k]) if k + step < len(x) else x[k] for k in range(keep)]
    r = pos & 31
    u = 31 - r
    hi = _shl(x[0], r) | _shr(_shr(x[1], 1), u)
    lo = _shl(x[1], r) | _shr(_shr(x[2], 1), u)
    w = []
    for i in range(4):
        view, n = hi, []
        for j in range(4):
            n.append(lax.clz(view))
            if j < 3:
                view = _shl(view, n[j] + 1)
        used = (n[0] + n[1]) + (n[2] + n[3]) + 4
        pos = pos + used
        if i < 3:
            hi = _shl(hi, used) | _shr(lo, 32 - used)
        if i < 2:
            lo = _shl(lo, used)
        q = _zeros_to_bin((n[0] | _shl(n[1], 8)) | (_shl(n[2], 16) | _shl(n[3], 24)))
        s = (signs if i == 0 else _shl(signs, i)) & MSB
        a, b = _swap_bytes(low[i], q | s)
        w += [bias - a, bias - b]
    return w, pos


MESH = pl.DeviceIdType.MESH
R = 256
LAG = 3
MSG_WORDS = 11
RAW, TRAILER = -1, -2


def make_kernel(NV=56, NIN=2, DS=3, DR=6, LY=1, CW=1024, post="axis1", vmem_mib=16, internal=None):
    def fn(x):
        m, n = x.shape
        half = m // 2
        NBLK = half // R
        NH = NBLK - NV
        TOTAL = NBLK + LAG

        def body(x_ref, h_ref, v_ref, in_buf, stage, tx_msg, tx_hdr, rx_msg, rx_hdr, win, pos,
                 load_sem, store_sem, tx_sem, fw_sem, rx_sem, raw_sem, credit):
            mx, my = lax.axis_index("x"), lax.axis_index("y")
            peer = ((mx, 1 - my), (1 - mx, my))
            in_base = (mx * half, (1 - mx) * half)
            quarter = (2 * my + mx, 2 * my + 1 - mx, 2 * (1 - my) + mx, 2 * (1 - my) + 1 - mx)

            def load(h, b):
                rows = pl.ds(pl.multiple_of(in_base[h] + b * R, R), R)
                return pltpu.make_async_copy(x_ref.at[rows], in_buf.at[h, b % NIN], load_sem.at[h, b % NIN])

            def on_result(s, b, f):
                @pl.when(b < NH)
                def _():
                    f(h_ref.at[quarter[s], pl.ds(pl.multiple_of(b * R, R), R)])

                @pl.when(b >= NH)
                def _():
                    f(v_ref.at[quarter[s], pl.ds(pl.multiple_of((b - NH) * R, R), R)])

            def store(s, b, act):
                on_result(s, b, lambda dst: act(pltpu.make_async_copy(stage.at[s, b % 2], dst, store_sem.at[s, b % 2])))

            start = lambda c: c.start()
            wait = lambda c: c.wait()
            wait_send = lambda c: c.wait_send()
            wait_recv = lambda c: c.wait_recv()

            def remote(src, dst, ssem, rsem, link):
                return pltpu.make_async_remote_copy(src, dst, ssem, rsem, device_id=peer[link], device_id_type=MESH)

            def hop(link, b):
                r = b % DR
                if link == 0:
                    s = b % DS
                    return tx_hdr.at[s], tx_msg.at[s], tx_sem.at[s], rx_hdr.at[0, r], rx_msg.at[0, r], rx_sem.at[0, r]
                return rx_hdr.at[0, r], rx_msg.at[0, r], fw_sem.at[r], rx_hdr.at[1, r], rx_msg.at[1, r], rx_sem.at[1, r]

            def header(link, b, act):
                sh, _, ss, dh, _, rs = hop(link, b)
                act(remote(sh, dh, ss.at[0], rs.at[0], link))

            def message(link, b, hdr, act):
                _, sm, ss, _, dm, rs = hop(link, b)
                for first in (0, 1):
                    for last in (MSG_WORDS, 2):
                        @pl.when(((b % 4 == 0) == (first == 1)) & ((hdr >= 0) == (last == MSG_WORDS)))
                        def _():
                            part = pl.ds(first, last - first)
                            act(remote(sm.at[part], dm.at[part], ss.at[1], rs.at[1], link))

            def raw(link, b, act):
                rsem = rx_sem.at[link, b % DR, 2]
                if link == 0:
                    on_result(0, b, lambda dst: act(remote(stage.at[0, b % 2], dst, raw_sem, rsem, 0)))
                else:
                    on_result(2, b, lambda dst: act(remote(dst, dst, raw_sem, rsem, 1)))

            def raw_arrival(link, b):
                rsem = rx_sem.at[link, b % DR, 2]
                on_result(2 + link, b, lambda dst: remote(stage.at[0, 0], dst, raw_sem, rsem, link).wait_recv())

            def start_and_drain(c):
                c.start()
                c.wait_send()

            def send(link, b, hdr):
                @pl.when(b >= DR)
                def _():
                    pl.semaphore_wait(credit.at[link], 1)
                header(link, b, start)
                message(link, b, hdr, start)

                @pl.when(hdr == RAW)
                def _():
                    raw(link, b, start_and_drain)

            def sent(link, b):
                hdr = jnp.max(hop(link, b)[0][...])
                header(link, b, wait_send)
                message(link, b, hdr, wait_send)

            def receive(link, b):
                header(link, b, wait_recv)
                hdr = jnp.max(rx_hdr[link, b % DR])
                message(link, b, hdr, wait_recv)

                @pl.when(hdr == RAW)
                def _():
                    raw_arrival(link, b)
                return hdr

            def first_bit(b):
                return (56 * b) & 31

            def code_words(b):
                return jnp.where(b % 4 == 0, 1, 2)

            col_groups = [pl.ds(c, CW) for c in range(0, n, CW)]

            def retire(b, keep):
                nb = code_words(b)
                s = b % DS
                for cols in col_groups:
                    words = [win[0, 2 + k, :, cols] for k in range(WORDS)]
                    p = pos[0, :, cols]
                    if keep is not None:
                        words = [w | jnp.where(keep, win[1, 2 + k, :, cols], 0) for k, w in enumerate(words)]
                        p = jnp.where(keep, pos[3, :, cols], p)
                    tx_msg[s, 0, :, cols] = words[0]
                    tx_msg[s, 1, :, cols] = jnp.where(nb == 1, words[0], words[1])
                    win[0, 7, :, cols] = jnp.zeros_like(p)
                    win[0, 8, :, cols] = jnp.zeros_like(p)
                    for k, w in enumerate(words):
                        win[0, 2 + k - nb, :, cols] = w
                    pos[0, :, cols] = jnp.maximum(p - 32 * nb, first_bit(b + 1))

            def encode(b):
                src, dst, s = in_buf.at[0, b % NIN], stage.at[0, b % 2], b % DS
                w0 = pltpu.bitcast(src[0:16, :].astype(jnp.bfloat16), jnp.int32)
                mags = (w0 & 0x7FFF) + (_shr(w0, 16) & 0x7FFF)
                top = (jnp.sum(mags) // (16 * n) + 517) & 0x7FFF
                bias = (top | 0x8000) | ((top | 0x8000) << 16)
                bad = None
                for cols in col_groups:
                    p = pos[0, :, cols]
                    for u in range(2):
                        w = []
                        for j in range(8 * u, 8 * u + 8):
                            xb = src[16 * j:16 * j + 16, cols].astype(jnp.bfloat16)
                            dst[16 * j:16 * j + 16, cols] = xb
                            w.append(pltpu.bitcast(xb, jnp.int32))
                        if u:
                            p = jnp.maximum(p, first_bit(b) + 28)
                        low, signs, z, p, bad_u = encode_unit(w, bias, p)
                        for k in range(4):
                            tx_msg[s, 3 + 4 * u + k, :, cols] = low[k]
                        if u == 0:
                            signs0, z0 = signs, z
                        bad = bad_u if bad is None else bad | bad_u
                    tx_msg[s, 2, :, cols] = signs0 | _shr(signs, 4)
                    for k in range(WORDS):
                        win[1, 2 + k, :, cols] = z0[k] | z[k]
                    pos[3, :, cols] = p
                fits = jnp.max(jnp.where(bad != 0, 1, 0)) == 0
                retire(b, fits)
                return jnp.where(fits, top, RAW)

            def decode(link, b):
                hdr = jnp.max(rx_hdr[link, b % DR])
                nb = code_words(b)

                @pl.when(hdr >= 0)
                def _():
                    bias = (hdr | 0x8000) | ((hdr | 0x8000) << 16)
                    dst = stage.at[2 + link, b % 2]
                    first = (56 * b) >> 5
                    where = []
                    for k in range(WORDS):
                        word = first + k
                        q, r = word // 7, word % 7
                        where.append(((4 * q + (r + 1) // 2) % DR, (r + 1) % 2))
                    msg = rx_msg.at[link, b % DR]
                    for cols in col_groups:
                        words = [rx_msg[link, s, j, :, cols] for s, j in where]
                        signs = msg[2, :, cols]
                        p = pos[1 + link, :, cols]
                        for u in range(2):
                            if u:
                                p = jnp.maximum(p, first_bit(b) + 28)
                                signs = signs << 4
                            w, p = decode_unit([msg[3 + 4 * u + k, :, cols] for k in range(4)], signs, words, bias, p)
                            for j in range(8):
                                rows = pl.ds(16 * (8 * u + j), 16)
                                dst[rows, cols] = pltpu.bitcast(w[j], jnp.bfloat16)
                        pos[1 + link, :, cols] = p
                    store(2 + link, b, start)
                pos[1 + link] = jnp.maximum(pos[1 + link] - 32 * nb, first_bit(b + 1))

            def decoded(link, b):
                @pl.when(jnp.max(rx_hdr[link, b % DR]) >= 0)
                def _():
                    store(2 + link, b, wait)

            def convert(b):
                src, dst = in_buf.at[1, b % NIN], stage.at[1, b % 2]
                for j in range(R // 64):
                    dst[64 * j:64 * j + 64, :] = src[64 * j:64 * j + 64, :].astype(jnp.bfloat16)

            for h in range(2):
                for b in range(NIN):
                    load(h, b).start()
            barrier = pltpu.get_barrier_semaphore()
            for p in peer:
                pl.semaphore_signal(barrier, 1, device_id=p, device_id_type=MESH)
            win[0] = jnp.zeros(win.shape[1:], jnp.int32)
            pos[...] = jnp.zeros(pos.shape, jnp.int32)

            def step(i, carry):
                @pl.when((i >= DS) & (i < TOTAL + DS))
                def _():
                    sent(0, i - DS)

                @pl.when((i >= 2) & (i < NBLK + 2))
                def _():
                    store(0, i - 2, wait)
                    store(1, i - 2, wait)

                @pl.when(i < NBLK)
                def _():
                    load(0, i).wait()
                    hdr = encode(i)
                    tx_hdr[i % DS] = jnp.full((1, 128), hdr, jnp.int32)
                    store(0, i, start)

                    @pl.when(i + NIN < NBLK)
                    def _():
                        load(0, i + NIN).start()

                @pl.when((i >= NBLK) & (i < TOTAL))
                def _():
                    retire(i, None)
                    tx_hdr[i % DS] = jnp.full((1, 128), TRAILER, jnp.int32)

                @pl.when(i == 0)
                def _():
                    pl.semaphore_wait(barrier, 2)

                @pl.when(i < TOTAL)
                def _():
                    send(0, i, jnp.max(tx_hdr[i % DS]))

                @pl.when(i < NBLK)
                def _():
                    load(1, i).wait()
                    convert(i)
                    store(1, i, start)

                    @pl.when(i + NIN < NBLK)
                    def _():
                        load(1, i + NIN).start()

                for link in range(2):
                    k = i - LY - link

                    @pl.when((k >= 0) & (k < TOTAL))
                    def _():
                        hdr = receive(link, k)
                        if link == 0:
                            send(1, k, hdr)

                    d = k - LAG

                    @pl.when((d >= 0) & (d < NBLK))
                    def _():
                        decode(link, d)

                    @pl.when((d >= 1) & (d <= NBLK))
                    def _():
                        decoded(link, d - 1)
                        if link == 0:
                            sent(1, d - 1)

                        @pl.when(d - 1 < TOTAL - DR)
                        def _():
                            pl.semaphore_signal(credit.at[link], 1, device_id=peer[link], device_id_type=MESH)
                return carry

            steps = TOTAL + LY + 2
            lax.fori_loop(0, steps, step, None)
            for b in range(max(steps - DS, 0), TOTAL):
                sent(0, jnp.int32(b))
            for b in range(NBLK, TOTAL):
                sent(1, jnp.int32(b))

        any_spec = pl.BlockSpec(memory_space=pl.ANY)
        i32 = jnp.int32
        h, v = pl.pallas_call(
            body,
            out_shape=(pltpu.HBM((4, NH * R, n), jnp.bfloat16), pltpu.VMEM((4, NV * R, n), jnp.bfloat16)),
            in_specs=[any_spec],
            out_specs=(any_spec, pl.BlockSpec(memory_space=pltpu.VMEM)),
            scratch_shapes=[
                pltpu.VMEM((2, NIN, R, n), jnp.float32),
                pltpu.VMEM((4, 2, R, n), jnp.bfloat16),
                pltpu.VMEM((DS, MSG_WORDS, 8, n), i32),
                pltpu.VMEM((DS, 1, 128), i32),
                pltpu.VMEM((2, DR, MSG_WORDS, 8, n), i32),
                pltpu.VMEM((2, DR, 1, 128), i32),
                pltpu.VMEM((2, 9, 8, n), i32),
                pltpu.VMEM((4, 8, n), i32),
                pltpu.SemaphoreType.DMA((2, NIN)),
                pltpu.SemaphoreType.DMA((4, 2)),
                pltpu.SemaphoreType.DMA((DS, 2)),
                pltpu.SemaphoreType.DMA((DR, 2)),
                pltpu.SemaphoreType.DMA((2, DR, 3)),
                pltpu.SemaphoreType.DMA,
                pltpu.SemaphoreType.REGULAR((2,)),
            ],
            compiler_params=pltpu.CompilerParams(collective_id=0, vmem_limit_bytes=vmem_mib * 2**20, internal_scratch_in_bytes=internal),
        )(x)
        if post == "axis1":
            return jnp.concatenate([h, v], axis=1).reshape(2 * m, n)
        return jnp.concatenate([p[q] for q in range(4) for p in (h, v)], axis=0)
    return fn


def pallas_dist_ag_xy_y_m65536_n1024_kernel(x: jax.Array):
    return make_kernel(DS=2)(x)
```

```python
import jax
import jax.numpy as jnp
import numpy as np
from jax import lax
from jax.experimental import pallas as pl
from jax.experimental.pallas import tpu as pltpu

ROWS = 256
BLOCK_BITS = 53
WINDOW = 8
LAG = 4
TAIL = 6
BIAS_OFFSET = 493
RAW = 0x8000
PLANES = 9
PIECES = (3, 3, 3)
EARLY = 2
TX_SLOTS = 2
RX_SLOTS = 6
RX_WORDS = 16
GROUP, IN_HBM = 16, 9
DRAIN = ((0, ()), (0, ()), (0, ()), (1, (0,)), (0, ()), (1, (1,)), (1, (2,)), (1, ()), (0, ()), (1, ()))


def _bytes(b):
    return np.uint32(b * 0x01010101).astype(np.int32)


def _shr(a, b):
    return lax.shift_right_logical(a, jnp.broadcast_to(jnp.asarray(b, jnp.int32), a.shape))


def _shl(a, b):
    return lax.shift_left(a, jnp.broadcast_to(jnp.asarray(b, jnp.int32), a.shape))


def _swap_bytes(a, b):
    t = (_shr(a, 8) ^ b) & 0x00FF00FF
    return a ^ _shl(t, 8), b ^ t


def _bin_to_length(q, low):
    ctx = _shr(low, 5) & _bytes(7)
    later = (q + ctx + _bytes(128 - 9)) & _bytes(128)
    top = (_bytes(128) - q) & _bytes(128)
    return q + _shr(later, 7) + ((top - _shr(top, 7)) & (_bytes(9) - ctx))


def _zeros_to_bin(zeros, low):
    t = zeros + (_shr(low, 5) & _bytes(7))
    later = (t + _bytes(128 - 9)) & _bytes(128)
    top = ((t + _bytes(128 - 8)) & _bytes(128)) ^ later
    return (zeros + _bytes(1) - _shr(later, 7)) & ~(top - _shr(top, 7))


def _encode(w, bias, pos):
    low, group, bits = [], [], []
    for i in range(4):
        lo, hi = _swap_bytes(bias - w[2 * i], bias - w[2 * i + 1])
        low.append(lo)
        sign = hi & _bytes(128)
        signs = sign if i == 0 else signs | _shr(sign, i)
        length = _bin_to_length(hi & _bytes(127), lo)
        longest = length if i == 0 else longest | length
        l0, l1, l2, l3 = (length & 31,) + tuple(_shr(length, s) & 31 for s in (8, 16, 24))
        code = _shl(jnp.ones_like(length), l1) | 1
        code = _shl(code, l2) | 1
        group.append(_shl(code, l3) | 1)
        bits.append((l0 + l1) + (l2 + l3))
    lo = group[0]
    for i in range(1, 4):
        carry = _shr(lo, -bits[i] & 31)
        hi = carry if i == 1 else _shl(hi, bits[i] & 31) | carry
        lo = _shl(lo, bits[i] & 31) | group[i]
    total = (bits[0] + bits[1]) + (bits[2] + bits[3])
    last = pos + total - 1
    misfit = ((longest & _bytes(0xE0)) | ((bits[0] | bits[1] | bits[2] | bits[3]) & -32)
              | ((total - 1) & -64) | (last & -(32 * WINDOW)))
    right = last & 31
    left = right ^ 31
    out = {-2: _shr(_shr(hi, 1), right), -1: _shl(hi, left) | _shr(_shr(lo, 1), right), 0: _shl(lo, left)}
    zero = jnp.zeros_like(lo)
    for step in (1, 2, 4):
        up = (last & (32 * step)) != 0
        out = {k: jnp.where(up, out.get(k - step, zero), out.get(k, zero))
               for k in range(0 if step == 4 else -2, max(out) + step + 1)}
    return low, signs, jnp.stack([out[k] for k in range(WINDOW)]), last + 1, misfit


def _decode(low, signs, window, bias, pos):
    x = list(window)
    for step, needed in ((4, 6), (2, 4), (1, 3)):
        down = (pos & (32 * step)) != 0
        x = [jnp.where(down, x[k + step], x[k]) if k + step < len(x) else x[k] for k in range(needed)]
    left = pos & 31
    right = left ^ 31
    hi = _shl(x[0], left) | _shr(_shr(x[1], 1), right)
    lo = _shl(x[1], left) | _shr(_shr(x[2], 1), right)
    w = []
    for i in range(4):
        view, zeros = hi, []
        for j in range(4):
            zeros.append(lax.clz(view))
            if j < 3:
                view = _shl(view, zeros[j] + 1)
        bits = (zeros[0] + zeros[1]) + (zeros[2] + zeros[3]) + 4
        pos = pos + bits
        if i < 3:
            hi = _shl(hi, bits) | _shr(lo, 32 - bits)
        if i < 2:
            lo = _shl(lo, bits)
        q = _zeros_to_bin((zeros[0] | _shl(zeros[1], 8)) | (_shl(zeros[2], 16) | _shl(zeros[3], 24)), low[i])
        sign = (_shl(signs, i) if i else signs) & _bytes(128)
        a, b = _swap_bytes(low[i], q | sign)
        w += [bias - a, bias - b]
    return w, pos


def _bias_word(header):
    half_word = (header & 0x7FFF) | 0x8000
    return half_word | (half_word << 16)


def _first_word(b):
    return (BLOCK_BITS * b) >> 5


def _first_bit(b):
    return (BLOCK_BITS * b) & 31


def _words_done(b):
    return _first_word(b + 1) - _first_word(b)


def _start(copy):
    copy.start()


def _wait(copy):
    copy.wait()


def _wait_send(copy):
    copy.wait_send()


def _wait_recv(copy):
    copy.wait_recv()


def _body(x_ref, hbm_out, vmem_out, in_buf, stage, tx_head, tx_code, tx_planes, rx_head, rx_code, rx_planes,
          window, pos, heads, load_sem, store_sem, send_sem, y_sem, x_sem, tail_sem, credit):
    half, n = x_ref.shape[0] // 2, x_ref.shape[1]
    blocks = half // ROWS
    mx, my = lax.axis_index("x"), lax.axis_index("y")
    peer = ((mx, 1 - my), (1 - mx, my))
    first_row = (mx * half, (1 - mx) * half)
    quarter = (2 * my + mx, 2 * my + 1 - mx, 2 * (1 - my) + mx, 2 * (1 - my) + 1 - mx)

    def part_rows(part, first=0):
        return pl.ds(first + part * (ROWS // 2), ROWS // 2)

    def load(s, b, part):
        rows = part_rows(part, pl.multiple_of(first_row[s] + b * ROWS, ROWS))
        return pltpu.make_async_copy(x_ref.at[rows], in_buf.at[s, part_rows(part)], load_sem.at[s, part])

    def start_load(s, b):
        for part in range(2):
            load(s, b, part).start()

    def with_result_rows(s, b, f):
        g, j = quarter[s] * (blocks // GROUP) + b // GROUP, b % GROUP
        pl.when(j < IN_HBM)(lambda: f(hbm_out.at[g, pl.ds(pl.multiple_of(j * ROWS, ROWS), ROWS)]))
        pl.when(j >= IN_HBM)(lambda: f(vmem_out.at[g, pl.ds(pl.multiple_of((j - IN_HBM) * ROWS, ROWS), ROWS)]))

    def store(s, b, act):
        with_result_rows(s, b, lambda rows: act(pltpu.make_async_copy(stage.at[s], rows, store_sem.at[s])))

    def remote(link, src, dst, src_sem, dst_sem):
        return pltpu.make_async_remote_copy(
            src, dst, src_sem, dst_sem, device_id=peer[link], device_id_type=pl.DeviceIdType.MESH)

    def arrival(link, b, k):
        return (y_sem, x_sem)[link].at[b % RX_SLOTS, k]

    def header(link, b, act):
        src = tx_head.at[b % TX_SLOTS] if link == 0 else rx_head.at[0, b % RX_SLOTS]
        act(remote(link, src, rx_head.at[link, b % RX_SLOTS], send_sem.at[link, b % RX_SLOTS, 0], arrival(link, b, 0)))

    def code(link, b, *acts):
        for j in range(2):
            @pl.when(j < _words_done(b))
            def _():
                word = (_first_word(b) + j) % RX_WORDS
                for hop, act in enumerate(acts, link):
                    src = tx_code.at[b % TX_SLOTS, j] if hop == 0 else rx_code.at[0, word]
                    act(remote(hop, src, rx_code.at[hop, word], send_sem.at[hop, b % RX_SLOTS, 1 + j],
                               arrival(hop, b, 1 + j)))

    def tail(link, head, *acts):
        for j in range(TAIL):
            @pl.when(j < (head >> 16))
            def _():
                word = (_first_word(blocks) + j) % RX_WORDS
                for hop, act in enumerate(acts, link):
                    src = window.at[2 + j] if hop == 0 else rx_code.at[0, word]
                    act(remote(hop, src, rx_code.at[hop, word], tail_sem.at[hop, 0, j], tail_sem.at[hop, 1, j]))

    def planes(link, b, begin, end, act):
        part = pl.ds(sum(PIECES[:begin]), sum(PIECES[begin:end]))
        src = tx_planes.at[b % TX_SLOTS, part] if link == 0 else rx_planes.at[0, b % RX_SLOTS, part]
        act(remote(link, src, rx_planes.at[link, b % RX_SLOTS, part], send_sem.at[link, b % RX_SLOTS, 3],
                   arrival(link, b, 3 + (begin if link == 0 else int(begin >= EARLY)))))

    def raw(link, b, stream, act):
        def f(rows):
            act(remote(link, stage.at[0] if link == 0 else rows, rows, send_sem.at[link, b % RX_SLOTS, 3],
                       arrival(link, b, 3)))
        with_result_rows(stream, b, f)

    def is_raw(who, b):
        return (heads[who, b % 8] & RAW) != 0

    def is_coded(who, b):
        return (heads[who, b % 8] & RAW) == 0

    def take_credit(link, b):
        pl.when(b >= RX_SLOTS)(lambda: pl.semaphore_wait(credit.at[link], 1))

    def encode(b):
        s = b % TX_SLOTS
        p = before = pos[0]
        for part in range(2):
            load(0, b, part).wait()
            value = in_buf[0, part_rows(part), :].astype(jnp.bfloat16)
            stage[0, part_rows(part), :] = value
            packed = pltpu.bitcast(value, jnp.int32)
            w = [packed[8 * j:8 * j + 8] for j in range(8)]
            if part == 0:
                head = (jnp.sum((w[0] & 0x7FFF) + (_shr(w[0], 16) & 0x7FFF)) // (16 * n) + BIAS_OFFSET) & 0x7FFF
            low, signs, codes, p, misfit = _encode(w, _bias_word(head), p)
            tx_planes[s, pl.ds(1 + 4 * part, 4)] = jnp.stack(low)
            if part == 0:
                first_signs, first_codes, first_misfit = signs, codes, misfit
        tx_planes[s, 0] = first_signs | _shr(signs, 4)
        fits = jnp.max(jnp.where((first_misfit | misfit) != 0, 1, 0)) == 0
        words = window[pl.ds(2, WINDOW)] | jnp.where(fits, first_codes | codes, 0)
        done = _words_done(b)
        tx_code[s] = words[:2]
        window[pl.ds(WINDOW, 2)] = jnp.zeros_like(words[:2])
        window[pl.ds(2 - done, WINDOW)] = words
        pos[0] = jnp.maximum(jnp.where(fits, p, before) - 32 * done, _first_bit(b + 1))
        return jnp.where(fits, head, RAW)

    def staged(b):
        store(0, b, _wait)
        pl.when(is_raw(0, b))(lambda: raw(0, b, 0, _wait_send))

    def sent(link, b):
        header(link, b, _wait_send)
        code(link, b, _wait_send)
        pl.when(is_coded(link, b))(lambda: planes(link, b, 0, len(PIECES), _wait_send))
        if link == 1:
            pl.when(is_raw(1, b))(lambda: raw(1, b, 2, _wait_send))

    def produce(b):
        pl.when(b >= 1)(lambda: staged(b - 1))
        pl.when(b >= TX_SLOTS)(lambda: sent(0, b - TX_SLOTS))
        heads[0, b % 8] = encode(b)

        @pl.when(b == blocks - 1)
        def _():
            heads[0, b % 8] |= ((jnp.max(pos[0]) + 31) >> 5) << 16

        tx_head[b % TX_SLOTS] = jnp.full((1, 128), heads[0, b % 8], jnp.int32)
        pl.when(b == 0)(lambda: pl.semaphore_wait(barrier, 2))
        take_credit(0, b)
        header(0, b, _start)
        code(0, b, _start)
        pl.when(b == blocks - 1)(lambda: tail(0, heads[0, b % 8], _start))
        pl.when(is_raw(0, b))(lambda: raw(0, b, 0, _start))

        @pl.when(is_coded(0, b))
        def _():
            for piece in range(len(PIECES)):
                planes(0, b, piece, piece + 1, _start)

        pl.when(b + 1 < blocks)(lambda: start_load(0, b + 1))
        store(0, b, _start)

    def keep(b):
        pl.when(b >= 1)(lambda: store(1, b - 1, _wait))
        for part in range(2):
            load(1, b, part).wait()
        stage[1] = in_buf[1].astype(jnp.bfloat16)
        store(1, b, _start)
        pl.when(b + 1 < blocks)(lambda: start_load(1, b + 1))

    def receive_header(link, b):
        header(link, b, _wait_recv)
        heads[1 + link, b % 8] = jnp.max(rx_head[link, b % RX_SLOTS])

    def relay_code(b):
        take_credit(1, b)
        receive_header(0, b)
        header(1, b, _start)
        code(0, b, _wait_recv, _start)

    def relay(b, piece):
        @pl.when(is_coded(1, b))
        def _():
            planes(0, b, piece, piece + 1, _wait_recv)
            planes(1, b, piece, piece + 1, _start)

        if piece == 0:
            @pl.when(is_raw(1, b))
            def _():
                raw(0, b, 2, _wait_recv)
                raw(1, b, 2, _start)

    def receive_code(b):
        receive_header(1, b)
        code(1, b, _wait_recv)

    def stored(link, b):
        pl.when(is_coded(1 + link, b))(lambda: store(2 + link, b, _wait))

    def consume(link, b):
        pl.when(b >= 1)(lambda: stored(link, b - 1))

        @pl.when(is_coded(1 + link, b))
        def _():
            s = b % RX_SLOTS
            words = [rx_code[link, (_first_word(b) + k) % RX_WORDS] for k in range(WINDOW)]
            bias = _bias_word(heads[1 + link, b % 8])
            p = pos[1 + link]
            for part, pieces in enumerate(((0, EARLY), (EARLY, len(PIECES)))):
                if link == 1:
                    planes(1, b, *pieces, _wait_recv)
                low = rx_planes[link, s, pl.ds(1 + 4 * part, 4)]
                w, p = _decode(low, rx_planes[link, s, 0] << (4 * part), words, bias, p)
                stage[2 + link, part_rows(part), :] = pltpu.bitcast(jnp.concatenate(w), jnp.bfloat16)
            pos[1 + link] = p
            store(2 + link, b, _start)

        pos[1 + link] = jnp.maximum(pos[1 + link] - 32 * _words_done(b), _first_bit(b + 1))
        if link == 0:
            pl.when(b < blocks - 1)(lambda: sent(1, b))
        else:
            pl.when(is_raw(2, b))(lambda: raw(1, b, 3, _wait_recv))

        @pl.when(b < blocks - RX_SLOTS)
        def _():
            pl.semaphore_signal(credit.at[link], 1, device_id=peer[link], device_id_type=pl.DeviceIdType.MESH)

    start_load(0, 0)
    barrier = pltpu.get_barrier_semaphore()
    for device in peer:
        pl.semaphore_signal(barrier, 1, device_id=device, device_id_type=pl.DeviceIdType.MESH)
    window[...] = jnp.zeros(window.shape, jnp.int32)
    pos[...] = jnp.zeros(pos.shape, jnp.int32)

    def step(i, carry):
        k, d = i - 1, i - 1 - LAG
        pl.when(k >= 0)(lambda: relay_code(k))
        produce(i)
        pl.when(i == 0)(lambda: start_load(1, 0))
        pl.when(k >= 0)(lambda: relay(k, 0))
        pl.when(d >= 0)(lambda: consume(0, d))
        pl.when(k >= 0)(lambda: keep(k))
        pl.when(k >= 0)(lambda: relay(k, 1))
        pl.when(k >= 0)(lambda: relay(k, 2))
        pl.when(k >= 0)(lambda: receive_code(k))
        pl.when(d >= 0)(lambda: consume(1, d))
        for piece in range(3, len(PIECES)):
            pl.when(k >= 0)(lambda: relay(k, piece))
        return carry

    lax.fori_loop(0, blocks, step, 0)

    last = jnp.int32(blocks - 1)
    relay_code(last)
    on_x = sum(link << j for j, (link, _) in enumerate(DRAIN))

    def drain(j, due):
        link = (on_x >> j) & 1

        @pl.when(j == 1)
        def _():
            keep(last)
            tail(0, heads[1, last % 8], _wait_recv, _start)

        for at, (_, pieces) in enumerate(DRAIN):
            for piece in pieces:
                pl.when(j == at)(lambda: relay(last, piece))

        @pl.when(link == 0)
        def _():
            consume(0, due[0])

        @pl.when(link == 1)
        def _():
            pl.when(due[1] == last - LAG)(lambda: receive_code(last))
            pl.when(due[1] == last - LAG + 1)(lambda: tail(1, heads[2, last % 8], _wait_recv))
            consume(1, due[1])

        return due[0] + 1 - link, due[1] + link

    lax.fori_loop(0, len(DRAIN), drain, (last - LAG, last - LAG))

    for b in range(blocks - TX_SLOTS, blocks):
        sent(0, jnp.int32(b))
    sent(1, last)
    staged(last)
    store(1, last, _wait)
    for link in range(2):
        tail(link, heads[link, last % 8], _wait_send)
        stored(link, last)


def pallas_dist_ag_xy_y_m65536_n1024_kernel(x: jax.Array):
    m, n = x.shape
    groups = 2 * m // (GROUP * ROWS)
    anywhere = pl.BlockSpec(memory_space=pl.ANY)
    pieces = pl.pallas_call(
        _body,
        out_shape=(jax.ShapeDtypeStruct((groups, IN_HBM * ROWS, n), jnp.bfloat16),
                   jax.ShapeDtypeStruct((groups, (GROUP - IN_HBM) * ROWS, n), jnp.bfloat16)),
        in_specs=[anywhere],
        out_specs=(anywhere, anywhere),
        scratch_shapes=[
            pltpu.VMEM((2, ROWS, n), jnp.float32),
            pltpu.VMEM((4, ROWS, n), jnp.bfloat16),
            pltpu.VMEM((TX_SLOTS, 1, 128), jnp.int32),
            pltpu.VMEM((TX_SLOTS, 2, 8, n), jnp.int32),
            pltpu.VMEM((TX_SLOTS, PLANES, 8, n), jnp.int32),
            pltpu.VMEM((2, RX_SLOTS, 1, 128), jnp.int32),
            pltpu.VMEM((2, RX_WORDS, 8, n), jnp.int32),
            pltpu.VMEM((2, RX_SLOTS, PLANES, 8, n), jnp.int32),
            pltpu.VMEM((WINDOW + 2, 8, n), jnp.int32),
            pltpu.VMEM((3, 8, n), jnp.int32),
            pltpu.SMEM((3, 8), jnp.int32),
            pltpu.SemaphoreType.DMA((2, 2)),
            pltpu.SemaphoreType.DMA((4,)),
            pltpu.SemaphoreType.DMA((2, RX_SLOTS, 4)),
            pltpu.SemaphoreType.DMA((RX_SLOTS, 3 + len(PIECES))),
            pltpu.SemaphoreType.DMA((RX_SLOTS, 5)),
            pltpu.SemaphoreType.DMA((2, 2, TAIL)),
            pltpu.SemaphoreType.REGULAR((2,)),
        ],
        compiler_params=pltpu.CompilerParams(collective_id=0, vmem_limit_bytes=16 * 2**20),
    )(x)

    strips = [p.reshape(groups, -1, 8, 4, n // 4).transpose(0, 1, 3, 2, 4).reshape(groups, -1, 8, n // 4)
              for p in pieces]
    out = jnp.concatenate(strips, axis=1)
    return out.reshape(groups, -1, 4, 8, n // 4).transpose(0, 1, 3, 2, 4).reshape(2 * m, n)
```
